```python
import numpy as np

kernel_name = "dist_ag_xy_y_m1024_n512"

def setup_inputs():
    return {"x": np.random.randn(2048, 512).astype(np.float32)}

def reference(x: np.ndarray) -> np.ndarray:
    return x
```

```python
import jax
import jax.numpy as jnp
from jax import lax
from jax.experimental import pallas as pl
from jax.experimental.pallas import tpu as pltpu

_MESH = pl.DeviceIdType.MESH

_F0 = 464
_F1 = 480
_PIECE = {0: 32, 1: 16}
_LOAD_ROWS = (16, 32, 128)


def _split(start, total, size):
    out = []
    r = start
    while r < start + total:
        s = min(size, start + total - r)
        out.append((r, s))
        r += s
    return out


def _compiler_params():
    try:
        return pltpu.CompilerParams(collective_id=0,
                                    disable_semaphore_checks=True)
    except TypeError:
        return pltpu.CompilerParams(collective_id=0)


def pallas_dist_ag_xy_y_m1024_n512_kernel(
x: jax.Array,
):
    m, n = x.shape
    f0, f1 = _F0, _F1
    e = m - f0 - f1
    assert e > 0 and f0 % 16 == 0 and f1 % 16 == 0 and m % 16 == 0

    relay_rng = {0: (0, f1), 1: (m - f0, f0)}
    own_only = {0: (m - f0, f0), 1: (0, f1)}
    sent_rng = {0: (0, f1 + e), 1: (f1, e + f0)}
    pieces = {c: _split(*relay_rng[c], _PIECE[c]) for c in (0, 1)}

    def load_groups(col):
        groups = []
        for start, total in (relay_rng[col], (f1, e)):
            r = start
            while r < start + total:
                i = len(groups)
                cap = _LOAD_ROWS[i] if i < len(_LOAD_ROWS) else m
                s = min(cap, start + total - r)
                groups.append((r, s))
                r += s
        groups.append(own_only[col])
        return groups

    groups_by_col = {c: load_groups(c) for c in (0, 1)}
    n_load = max(len(g) for g in groups_by_col.values())
    n_yrecv = max(len(p) for p in pieces.values()) + 1

    def body(x_ref, out_ref, xin, lsem, ysend, yrecv, xsend, xrecv, xready):
        my_x = lax.axis_index("x")
        my_y = lax.axis_index("y")
        ynbr = (my_x, 1 - my_y)
        xnbr = (1 - my_x, my_y)
        mine = pl.multiple_of(my_y * m, m)
        theirs = pl.multiple_of((1 - my_y) * m, m)
        barrier = pltpu.get_barrier_semaphore()

        def rcopy(base, r, s, send_sem, recv_sem, dev):
            rows = out_ref.at[pl.ds(base + r, s)]
            return pltpu.make_async_remote_copy(
                src_ref=rows, dst_ref=rows, send_sem=send_sem,
                recv_sem=recv_sem, device_id=dev, device_id_type=_MESH)

        def column(col):
            groups = groups_by_col[col]
            mine_pieces = pieces[col]
            n_send_groups = len(groups) - 1

            def load(g):
                r, s = groups[g]
                return pltpu.make_async_copy(
                    x_ref.at[pl.ds(r, s)], xin.at[pl.ds(r, s)], lsem.at[g])

            def round_rows(g):
                r, s = groups[g]
                out_ref[pl.ds(mine + r, s), :] = (
                    xin[pl.ds(r, s), :].astype(out_ref.dtype))

            load(0).start()
            load(1).start()

            pl.semaphore_signal(barrier, inc=1, device_id=ynbr,
                                device_id_type=_MESH)
            if col == 0:
                pl.semaphore_signal(barrier, inc=1, device_id=xnbr,
                                    device_id_type=_MESH)

            k = 0
            for g in range(n_send_groups):
                load(g).wait()
                if g + 2 <= n_send_groups:
                    load(g + 2).start()
                round_rows(g)
                if g == 0:
                    pl.semaphore_wait(barrier, 1 if col == 0 else 2)
                g0, gs = groups[g]
                while (k < len(mine_pieces)
                       and g0 < sum(mine_pieces[k]) <= g0 + gs):
                    r, s = mine_pieces[k]
                    rcopy(mine, r, s, ysend, yrecv.at[k], ynbr).start()
                    k += 1
                if g == 0 and col == 1:
                    pl.semaphore_signal(xready, inc=1, device_id=xnbr,
                                        device_id_type=_MESH)
            assert k == len(mine_pieces)
            rcopy(mine, f1, e, ysend, yrecv.at[k], ynbr).start()

            if col == 0:
                pl.semaphore_wait(xready, 1)
            for k, (r, s) in enumerate(mine_pieces):
                rcopy(theirs, r, s, ysend, yrecv.at[k], ynbr).wait_recv()
                rcopy(theirs, r, s, xsend, xrecv, xnbr).start()

            load(n_send_groups).wait()
            round_rows(n_send_groups)

            rcopy(theirs, f1, e, ysend, yrecv.at[len(mine_pieces)],
                  ynbr).wait_recv()
            rcopy(theirs, *relay_rng[1 - col], xsend, xrecv, xnbr).wait_recv()
            rcopy(mine, *sent_rng[col], ysend, yrecv.at[0], ynbr).wait_send()
            rcopy(theirs, *relay_rng[col], xsend, xrecv, xnbr).wait_send()

        @pl.when(my_x == 0)
        def _():
            column(0)

        @pl.when(my_x == 1)
        def _():
            column(1)

    return pl.pallas_call(
        body,
        out_shape=jax.ShapeDtypeStruct((2 * m, n), jnp.bfloat16),
        in_specs=[pl.BlockSpec(memory_space=pl.ANY)],
        out_specs=pl.BlockSpec(memory_space=pltpu.VMEM),
        scratch_shapes=[
            pltpu.VMEM((m, n), x.dtype),
            pltpu.SemaphoreType.DMA((n_load,)),
            pltpu.SemaphoreType.DMA,
            pltpu.SemaphoreType.DMA((n_yrecv,)),
            pltpu.SemaphoreType.DMA,
            pltpu.SemaphoreType.DMA,
            pltpu.SemaphoreType.REGULAR,
        ],
        compiler_params=_compiler_params(),
    )(x)
```
